```python
import numpy as np

kernel_name = "dist_max_ax1_xy_m4096_n1024"

def setup_inputs():
    return {"x": np.random.randn(8192, 2048).astype(np.float32)}

def reference(x: np.ndarray) -> np.ndarray:
    return np.max(x, axis=1, keepdims=True)
```

```python
import jax
import jax.numpy as jnp
from jax import lax
from jax.experimental import pallas as pl
from jax.experimental.pallas import tpu as pltpu

M, N = 4096, 1024
H = M // 2
G = H // 128

EARLY = (2048,)
LATE = (1024, 512, 256, 128, 128)
NFIN = (15, 1)


def _rowmax128(blk):
    m = blk[:, 0:128]
    for c in range(1, N // 128):
        m = jnp.maximum(m, blk[:, c * 128:(c + 1) * 128])
    return jnp.max(m.T, axis=0, keepdims=True)


def pallas_dist_max_ax1_xy_m4096_n1024_kernel(x: jax.Array):
    chunks = list(EARLY) + list(LATE)
    offs = [sum(chunks[:i]) for i in range(len(chunks))]
    nch = len(chunks)

    def body(x_hbm, out_ref, buf, part, recv, in_sems, send_sems, recv_sems):
        my_x = lax.axis_index("x")
        my_y = lax.axis_index("y")
        peer = (my_x, 1 - my_y)

        def cp(i):
            o = offs[i]
            if o < H:
                src = (1 - my_y) * H + o
            else:
                src = my_y * H + (o - H)
            src = pl.multiple_of(src, 128)
            return pltpu.make_async_copy(
                x_hbm.at[pl.ds(src, chunks[i])],
                buf.at[pl.ds(o, chunks[i])],
                in_sems.at[i],
            )

        cp(0).start()
        bar = pltpu.get_barrier_semaphore()
        pl.semaphore_signal(bar, inc=1, device_id=peer,
                            device_id_type=pl.DeviceIdType.MESH)
        for i in range(1, nch):
            cp(i).start()

        def rcopy(src, dst, k):
            return pltpu.make_async_remote_copy(
                src, dst, send_sems.at[k], recv_sems.at[k],
                device_id=peer, device_id_type=pl.DeviceIdType.MESH)

        rd_part = rcopy(part, recv, 0)
        fin = []
        g0 = 0
        for k, n in enumerate(NFIN):
            mine = out_ref.at[my_y, pl.ds(g0, n)]
            theirs = out_ref.at[1 - my_y, pl.ds(g0, n)]
            fin.append((g0, n, rcopy(mine, mine, 1 + k),
                        rcopy(theirs, theirs, 1 + k)))
            g0 += n

        for i in range(len(EARLY)):
            cp(i).wait()

            def ebody(r, carry):
                row0 = pl.multiple_of(offs[i] + r * 128, 128)
                part[pl.ds(offs[i] // 128 + r, 1), :] = _rowmax128(
                    buf[pl.ds(row0, 128), :])
                return carry

            lax.fori_loop(0, chunks[i] // 128, ebody, 0)
        pl.semaphore_wait(bar, 1)
        rd_part.start()
        for i in range(len(EARLY), nch):
            cp(i).wait()
            if i == len(EARLY):
                rd_part.wait_recv()
            for r in range(chunks[i] // 128):
                g = (offs[i] - H) // 128 + r
                v = _rowmax128(buf[pl.ds(offs[i] + r * 128, 128), :])
                out_ref[my_y, pl.ds(g, 1), :] = jnp.maximum(
                    v, recv[pl.ds(g, 1), :])
                for (g0, n, snd, rcv) in fin:
                    if g == g0 + n - 1:
                        snd.start()
        rd_part.wait_send()
        for (g0, n, snd, rcv) in fin:
            snd.wait_send()
        for (g0, n, snd, rcv) in fin:
            rcv.wait_recv()

    out = pl.pallas_call(
        body,
        out_shape=jax.ShapeDtypeStruct((2, G, 128), jnp.float32),
        in_specs=[pl.BlockSpec(memory_space=pl.ANY)],
        out_specs=pl.BlockSpec(memory_space=pltpu.VMEM),
        scratch_shapes=[
            pltpu.VMEM((M, N), jnp.float32),
            pltpu.VMEM((G, 128), jnp.float32),
            pltpu.VMEM((G, 128), jnp.float32),
            pltpu.SemaphoreType.DMA((nch,)),
            pltpu.SemaphoreType.DMA((1 + len(NFIN),)),
            pltpu.SemaphoreType.DMA((1 + len(NFIN),)),
        ],
        compiler_params=pltpu.CompilerParams(
            collective_id=0, vmem_limit_bytes=64 * 1024 * 1024),
    )(x)
    return out.reshape(M, 1)
```

```python
import jax
import jax.numpy as jnp
from jax import lax
from jax.experimental import pallas as pl
from jax.experimental.pallas import tpu as pltpu

M, N = 4096, 1024
H = M // 2
G = H // 128
NEG = float("-inf")
MESH = pl.DeviceIdType.MESH

RB = 64
S = 96
XB = 48
EC = 2
LAST = (96, 32)
S_FWD_AT = 11
XA_AT, RA_AT, XB_AT, S_AT, RB_AT, XRET_AT = 7, 7, 11, 12, 13, 14


def _tree_max(parts):
    while len(parts) > 1:
        nxt = [jnp.maximum(parts[i], parts[i + 1])
               for i in range(0, len(parts) - 1, 2)]
        if len(parts) % 2:
            nxt.append(parts[-1])
        parts = nxt
    return parts[0]


def _place(blk, lane0):
    r = blk.shape[0]
    m = _tree_max([blk[:, c * 128:(c + 1) * 128] for c in range(N // 128)])
    v = jnp.max(m, axis=1, keepdims=True)
    lane = lax.broadcasted_iota(jnp.int32, (r, 128), 1)
    row = lax.broadcasted_iota(jnp.int32, (r, 128), 0)
    sel = jnp.where(lane == row + lane0, v, NEG)
    return _tree_max([sel[j * 8:(j + 1) * 8] for j in range(r // 8)])


def _rowmax(blk, lane0=0):
    return jnp.max(_place(blk, lane0), axis=0, keepdims=True)


def pallas_dist_max_ax1_xy_m4096_n1024_kernel(x: jax.Array):
    early = [(128 + RB, 128 - RB)] + [(o, 128 * EC) for o in range(256, H, 128 * EC)]
    irr = [(0, 256), (256 + S, 128 - S), (512 + XB, 128 - XB)]
    reg = [(o, 128) for o in range(640, H - 128, 128)]
    lastc = [(H - 128 + sum(LAST[:i]), c) for i, c in enumerate(LAST)]
    ne, ni, nr = len(early), len(irr), len(reg)
    nch = ne + ni + nr + len(lastc)

    def body(x_hbm, out_ref, buf, xbuf, sm, part, recv, xpart, xrecv,
             in_sems, sm_sems, send_sems, recv_sems):
        my_x = lax.axis_index("x")
        my_y = lax.axis_index("y")
        yp = (my_x, 1 - my_y)
        xp = (1 - my_x, my_y)
        ebase = (1 - my_y) * H
        lbase = my_y * H

        def src(base, o, n):
            return x_hbm.at[pl.ds(pl.multiple_of(base + o, 8), n)]

        def ecp(i, o, c):
            return pltpu.make_async_copy(
                src(ebase, o, c), buf.at[pl.ds(pl.multiple_of(o, 8), c)],
                in_sems.at[i])

        def lcp(i, o, c):
            return pltpu.make_async_copy(
                src(lbase, o, c), buf.at[pl.ds(pl.multiple_of(H + o, 8), c)],
                in_sems.at[i])

        def rcopy(s, d, k, dev):
            return pltpu.make_async_remote_copy(
                s, d, send_sems.at[k], recv_sems.at[k],
                device_id=dev, device_id_type=MESH)

        ecp(0, *early[0]).start()
        ecp(1, *early[1]).start()
        s_in = pltpu.make_async_copy(src(lbase, 256, S), sm, sm_sems.at[0])
        s_out = pltpu.make_async_copy(sm, buf.at[pl.ds(H + 256, S)], sm_sems.at[1])
        s_in.start()
        bar = pltpu.get_barrier_semaphore()
        pl.semaphore_signal(bar, inc=1, device_id=yp, device_id_type=MESH)
        pl.semaphore_signal(bar, inc=1, device_id=xp, device_id_type=MESH)
        for i in range(2, ne):
            ecp(i, *early[i]).start()
        for j, (o, c) in enumerate(irr + reg + lastc):
            lcp(ne + j, o, c).start()

        rd_part = rcopy(part.at[pl.ds(1, G - 1)], recv.at[pl.ds(1, G - 1)], 0, yp)
        fin = []
        for k, (g0, n) in enumerate([(0, G - 1), (G - 1, 1)]):
            own = out_ref.at[my_y, pl.ds(g0, n)]
            oth = out_ref.at[1 - my_y, pl.ds(g0, n)]
            fin.append((rcopy(own, own, 1 + k, yp), rcopy(oth, oth, 1 + k, yp)))
        r_a = rcopy(src(ebase, 0, 128), buf.at[pl.ds(0, 128)], 3, yp)
        r_b = rcopy(src(ebase, 128, RB), buf.at[pl.ds(128, RB)], 4, yp)
        x_a = rcopy(src(lbase, 384, 128), xbuf.at[pl.ds(0, 128)], 5, xp)
        x_b = rcopy(src(lbase, 512, XB), xbuf.at[pl.ds(128, XB)], 6, xp)
        x_r = rcopy(xpart, xrecv, 7, xp)

        pl.semaphore_wait(bar, 2)
        r_a.start()
        x_a.start()
        x_b.start()

        ecp(0, *early[0]).wait()
        part[pl.ds(1, 1), :] = _rowmax(buf[pl.ds(early[0][0], early[0][1]), :], RB)

        def eloop(lo, hi):
            def step(i, carry):
                o = pl.multiple_of(256 + (i - 1) * 128 * EC, 128)
                ecp(i, o, 128 * EC).wait()
                for r in range(EC):
                    row0 = pl.multiple_of(o + r * 128, 128)
                    part[pl.ds(2 + (i - 1) * EC + r, 1), :] = _rowmax(
                        buf[pl.ds(row0, 128), :])
                return carry
            lax.fori_loop(lo, hi, step, 0)

        mid = 1 + (S_FWD_AT - 1) // EC
        eloop(1, mid)
        s_in.wait()
        s_out.start()
        eloop(mid, ne)
        rd_part.start()
        r_b.start()

        mine = out_ref.at[my_y]

        def merge(g, v):
            mine[pl.ds(g, 1), :] = jnp.maximum(mine[pl.ds(g, 1), :], v)

        mine[pl.ds(3, 1), :] = jnp.full((1, 128), NEG, jnp.float32)
        for j, (o, c) in enumerate(irr):
            lcp(ne + j, o, c).wait()
            for r in range(max(1, c // 128)):
                mine[pl.ds(o // 128 + r, 1), :] = _rowmax(
                    buf[pl.ds(H + o + r * 128, min(c, 128)), :], o % 128)

        def lloop(g_lo, g_hi):
            def step(g, carry):
                o = pl.multiple_of(g * 128, 128)
                lcp(ne + ni + g - 5, o, 128).wait()
                mine[pl.ds(g, 1), :] = _rowmax(
                    buf[pl.ds(pl.multiple_of(H + o, 128), 128), :])
                return carry
            if g_hi > g_lo:
                lax.fori_loop(g_lo, g_hi, step, 0)

        def ev_xa():
            x_a.wait_recv()
            xpart[pl.ds(0, 1), :] = _rowmax(xbuf[pl.ds(0, 128), :])

        def ev_xb():
            x_b.wait_recv()
            xpart[pl.ds(1, 1), :] = _rowmax(xbuf[pl.ds(128, XB), :])
            x_r.start()

        def ev_ra():
            r_a.wait_recv()
            merge(0, _rowmax(buf[pl.ds(0, 128), :]))

        def ev_rb():
            r_b.wait_recv()
            merge(1, _rowmax(buf[pl.ds(128, RB), :]))

        def ev_s():
            s_out.wait()
            merge(2, _rowmax(buf[pl.ds(H + 256, S), :]))

        def ev_xr():
            x_r.wait_recv()
            mine[pl.ds(3, 2), :] = jnp.maximum(mine[pl.ds(3, 2), :], xrecv[...])

        g = 5
        for at, fn in [(XA_AT, ev_xa), (RA_AT, ev_ra), (XB_AT, ev_xb),
                       (S_AT, ev_s), (RB_AT, ev_rb), (XRET_AT, ev_xr)]:
            lloop(g, at + 1)
            g = max(g, at + 1)
            fn()
        lloop(g, G - 1)

        rd_part.wait_recv()
        mine[pl.ds(1, G - 2), :] = jnp.maximum(
            mine[pl.ds(1, G - 2), :], recv[pl.ds(1, G - 2), :])
        fin[0][0].start()

        acc = jnp.broadcast_to(recv[pl.ds(G - 1, 1), :], (8, 128))
        for j, (o, c) in enumerate(lastc):
            lcp(ne + ni + nr + j, o, c).wait()
            acc = jnp.maximum(acc, _place(buf[pl.ds(H + o, c), :], o % 128))
        mine[pl.ds(G - 1, 1), :] = jnp.max(acc, axis=0, keepdims=True)
        fin[1][0].start()

        for s in (rd_part, r_a, r_b, x_a, x_b, x_r, fin[0][0], fin[1][0]):
            s.wait_send()
        fin[0][1].wait_recv()
        fin[1][1].wait_recv()

    out = pl.pallas_call(
        body,
        out_shape=jax.ShapeDtypeStruct((2, G, 128), jnp.float32),
        in_specs=[pl.BlockSpec(memory_space=pl.ANY)],
        out_specs=pl.BlockSpec(memory_space=pltpu.VMEM),
        scratch_shapes=[
            pltpu.VMEM((M, N), jnp.float32),
            pltpu.VMEM((256, N), jnp.float32),
            pltpu.SMEM((S, N), jnp.float32),
            pltpu.VMEM((G, 128), jnp.float32),
            pltpu.VMEM((G, 128), jnp.float32),
            pltpu.VMEM((2, 128), jnp.float32),
            pltpu.VMEM((2, 128), jnp.float32),
            pltpu.SemaphoreType.DMA((nch,)),
            pltpu.SemaphoreType.DMA((2,)),
            pltpu.SemaphoreType.DMA((8,)),
            pltpu.SemaphoreType.DMA((8,)),
        ],
        compiler_params=pltpu.CompilerParams(
            collective_id=0,
            vmem_limit_bytes=64 * 1024 * 1024,
            disable_semaphore_checks=True,
            disable_bounds_checks=True,
        ),
    )(x)
    return out.reshape(M, 1)
```

```python
import jax
import jax.numpy as jnp
from jax import lax
from jax.experimental import pallas as pl
from jax.experimental.pallas import tpu as pltpu

M, N = 4096, 1024
H = M // 2
G = H // 128
NEG = float("-inf")
MESH = pl.DeviceIdType.MESH

RB = 64
S = 96
XB = 48
EC = 2
LAST = (96, 32)
S_FWD_AT = 11
X_AT, S_AT, R_AT, XRET_AT = 11, 12, 13, 14


def _tree_max(parts):
    while len(parts) > 1:
        nxt = [jnp.maximum(parts[i], parts[i + 1])
               for i in range(0, len(parts) - 1, 2)]
        if len(parts) % 2:
            nxt.append(parts[-1])
        parts = nxt
    return parts[0]


def _place(blk, lane0):
    r = blk.shape[0]
    m = _tree_max([blk[:, c * 128:(c + 1) * 128] for c in range(N // 128)])
    v = jnp.max(m, axis=1, keepdims=True)
    lane = lax.broadcasted_iota(jnp.int32, (r, 128), 1)
    row = lax.broadcasted_iota(jnp.int32, (r, 128), 0)
    sel = jnp.where(lane == row + lane0, v, NEG)
    return _tree_max([sel[j * 8:(j + 1) * 8] for j in range(r // 8)])


def _rowmax(blk, lane0=0):
    return jnp.max(_place(blk, lane0), axis=0, keepdims=True)


def pallas_dist_max_ax1_xy_m4096_n1024_kernel(x: jax.Array):
    early = [(128 + RB, 128 - RB)] + [(o, 128 * EC) for o in range(256, H, 128 * EC)]
    irr = [(0, 256), (256 + S, 128 - S), (512 + XB, 128 - XB)]
    reg = [(o, 128) for o in range(640, H - 128, 128)]
    lastc = [(H - 128 + sum(LAST[:i]), c) for i, c in enumerate(LAST)]
    ne, ni, nr = len(early), len(irr), len(reg)
    nch = ne + ni + nr + len(lastc)

    def body(x_hbm, out_ref, buf, xbuf, sm, part, recv, xpart, xrecv,
             in_sems, sm_sems, send_sems, recv_sems):
        my_x = lax.axis_index("x")
        my_y = lax.axis_index("y")
        yp = (my_x, 1 - my_y)
        xp = (1 - my_x, my_y)
        ebase = (1 - my_y) * H
        lbase = my_y * H

        def src(base, o, n):
            return x_hbm.at[pl.ds(pl.multiple_of(base + o, 8), n)]

        def ecp(i, o, c):
            return pltpu.make_async_copy(
                src(ebase, o, c), buf.at[pl.ds(pl.multiple_of(o, 8), c)],
                in_sems.at[i])

        def lcp(i, o, c):
            return pltpu.make_async_copy(
                src(lbase, o, c), buf.at[pl.ds(pl.multiple_of(H + o, 8), c)],
                in_sems.at[i])

        def rcopy(s, d, k, dev):
            return pltpu.make_async_remote_copy(
                s, d, send_sems.at[k], recv_sems.at[k],
                device_id=dev, device_id_type=MESH)

        ecp(0, *early[0]).start()
        ecp(1, *early[1]).start()
        s_in = pltpu.make_async_copy(src(lbase, 256, S), sm, sm_sems.at[0])
        s_out = pltpu.make_async_copy(sm, buf.at[pl.ds(H + 256, S)], sm_sems.at[1])
        s_in.start()
        bar = pltpu.get_barrier_semaphore()
        pl.semaphore_signal(bar, inc=1, device_id=yp, device_id_type=MESH)
        pl.semaphore_signal(bar, inc=1, device_id=xp, device_id_type=MESH)
        for i in range(2, ne):
            ecp(i, *early[i]).start()
        for j, (o, c) in enumerate(irr + reg + lastc):
            lcp(ne + j, o, c).start()

        y_raw = rcopy(src(ebase, 0, 128 + RB), buf.at[pl.ds(0, 128 + RB)], 0, yp)
        x_raw = rcopy(src(lbase, 384, 128 + XB), xbuf, 1, xp)
        y_part = rcopy(part.at[pl.ds(1, G - 1)], recv.at[pl.ds(1, G - 1)], 2, yp)
        x_ret = rcopy(xpart, xrecv, 3, xp)
        fin_send, fin_recv = [], []
        for k, (g0, n) in enumerate([(0, G - 1), (G - 1, 1)]):
            own = out_ref.at[my_y, pl.ds(g0, n)]
            oth = out_ref.at[1 - my_y, pl.ds(g0, n)]
            fin_send.append(rcopy(own, own, 4 + k, yp))
            fin_recv.append(rcopy(oth, oth, 4 + k, yp))

        pl.semaphore_wait(bar, 2)
        y_raw.start()
        x_raw.start()

        ecp(0, *early[0]).wait()
        part[pl.ds(1, 1), :] = _rowmax(buf[pl.ds(early[0][0], early[0][1]), :], RB)

        def eloop(lo, hi):
            def step(i, carry):
                o = pl.multiple_of(256 + (i - 1) * 128 * EC, 128)
                ecp(i, o, 128 * EC).wait()
                for r in range(EC):
                    row0 = pl.multiple_of(o + r * 128, 128)
                    part[pl.ds(2 + (i - 1) * EC + r, 1), :] = _rowmax(
                        buf[pl.ds(row0, 128), :])
                return carry
            lax.fori_loop(lo, hi, step, 0)

        mid = 1 + (S_FWD_AT - 1) // EC
        eloop(1, mid)
        s_in.wait()
        s_out.start()
        eloop(mid, ne)
        y_part.start()

        mine = out_ref.at[my_y]

        def merge(g, v):
            mine[pl.ds(g, 1), :] = jnp.maximum(mine[pl.ds(g, 1), :], v)

        mine[pl.ds(3, 1), :] = jnp.full((1, 128), NEG, jnp.float32)
        for j, (o, c) in enumerate(irr):
            lcp(ne + j, o, c).wait()
            for r in range(max(1, c // 128)):
                mine[pl.ds(o // 128 + r, 1), :] = _rowmax(
                    buf[pl.ds(H + o + r * 128, min(c, 128)), :], o % 128)

        def lloop(g_lo, g_hi):
            def step(g, carry):
                o = pl.multiple_of(g * 128, 128)
                lcp(ne + ni + g - 5, o, 128).wait()
                mine[pl.ds(g, 1), :] = _rowmax(
                    buf[pl.ds(pl.multiple_of(H + o, 128), 128), :])
                return carry
            lax.fori_loop(g_lo, g_hi, step, 0)

        lloop(5, X_AT + 1)
        x_raw.wait_recv()
        xpart[pl.ds(0, 1), :] = _rowmax(xbuf[pl.ds(0, 128), :])
        xpart[pl.ds(1, 1), :] = _rowmax(xbuf[pl.ds(128, XB), :])
        x_ret.start()

        lloop(X_AT + 1, S_AT + 1)
        s_out.wait()
        merge(2, _rowmax(buf[pl.ds(H + 256, S), :]))

        lloop(S_AT + 1, R_AT + 1)
        y_raw.wait_recv()
        merge(0, _rowmax(buf[pl.ds(0, 128), :]))
        merge(1, _rowmax(buf[pl.ds(128, RB), :]))

        lloop(R_AT + 1, XRET_AT + 1)
        x_ret.wait_recv()
        mine[pl.ds(3, 2), :] = jnp.maximum(mine[pl.ds(3, 2), :], xrecv[...])

        y_part.wait_recv()
        mine[pl.ds(1, G - 2), :] = jnp.maximum(
            mine[pl.ds(1, G - 2), :], recv[pl.ds(1, G - 2), :])
        fin_send[0].start()

        acc = jnp.broadcast_to(recv[pl.ds(G - 1, 1), :], (8, 128))
        for j, (o, c) in enumerate(lastc):
            lcp(ne + ni + nr + j, o, c).wait()
            acc = jnp.maximum(acc, _place(buf[pl.ds(H + o, c), :], o % 128))
        mine[pl.ds(G - 1, 1), :] = jnp.max(acc, axis=0, keepdims=True)
        fin_send[1].start()

        for s in (y_raw, x_raw, y_part, x_ret, fin_send[0], fin_send[1]):
            s.wait_send()
        fin_recv[0].wait_recv()
        fin_recv[1].wait_recv()

    assert XRET_AT == G - 2
    out = pl.pallas_call(
        body,
        out_shape=jax.ShapeDtypeStruct((2, G, 128), jnp.float32),
        in_specs=[pl.BlockSpec(memory_space=pl.ANY)],
        out_specs=pl.BlockSpec(memory_space=pltpu.VMEM),
        scratch_shapes=[
            pltpu.VMEM((M, N), jnp.float32),
            pltpu.VMEM((128 + XB, N), jnp.float32),
            pltpu.SMEM((S, N), jnp.float32),
            pltpu.VMEM((G, 128), jnp.float32),
            pltpu.VMEM((G, 128), jnp.float32),
            pltpu.VMEM((2, 128), jnp.float32),
            pltpu.VMEM((2, 128), jnp.float32),
            pltpu.SemaphoreType.DMA((nch,)),
            pltpu.SemaphoreType.DMA((2,)),
            pltpu.SemaphoreType.DMA((6,)),
            pltpu.SemaphoreType.DMA((6,)),
        ],
        compiler_params=pltpu.CompilerParams(
            collective_id=0,
            vmem_limit_bytes=64 * 1024 * 1024,
            disable_semaphore_checks=True,
            disable_bounds_checks=True,
        ),
    )(x)
    return out.reshape(M, 1)
```

```python
import jax
import jax.numpy as jnp
from jax import lax
from jax.experimental import pallas as pl
from jax.experimental.pallas import tpu as pltpu

M, N = 4096, 1024
H = M // 2
G = H // 128
NEG = float("-inf")
MESH = pl.DeviceIdType.MESH

RB = 80
S = 112
XB = 64
EC = 2
LAST = (96, 32)
S_FWD_AT = 11
X_AT, S_AT = 10, 13


def _tree_max(parts):
    while len(parts) > 1:
        nxt = [jnp.maximum(parts[i], parts[i + 1])
               for i in range(0, len(parts) - 1, 2)]
        if len(parts) % 2:
            nxt.append(parts[-1])
        parts = nxt
    return parts[0]


def _place(blk, lane0):
    r = blk.shape[0]
    m = _tree_max([blk[:, c * 128:(c + 1) * 128] for c in range(N // 128)])
    v = jnp.max(m, axis=1, keepdims=True)
    lane = lax.broadcasted_iota(jnp.int32, (r, 128), 1)
    row = lax.broadcasted_iota(jnp.int32, (r, 128), 0)
    sel = jnp.where(lane == row + lane0, v, NEG)
    return _tree_max([sel[j * 8:(j + 1) * 8] for j in range(r // 8)])


def _rowmax(blk, lane0=0):
    return jnp.max(_place(blk, lane0), axis=0, keepdims=True)


def pallas_dist_max_ax1_xy_m4096_n1024_kernel(x: jax.Array):
    early = [(128 + RB, 128 - RB)] + [(o, 128 * EC) for o in range(256, H, 128 * EC)]
    irr = [(0, 256), (256 + S, 128 - S), (512 + XB, 128 - XB)]
    reg = [(o, 128) for o in range(640, H - 128, 128)]
    lastc = [(H - 128 + sum(LAST[:i]), c) for i, c in enumerate(LAST)]
    ne, ni, nr = len(early), len(irr), len(reg)
    nch = ne + ni + nr + len(lastc)

    def body(x_hbm, out_ref, buf, xbuf, sm, part, recv, xpart, xrecv,
             in_sems, sm_sems, send_sems, recv_sems):
        my_x = lax.axis_index("x")
        my_y = lax.axis_index("y")
        yp = (my_x, 1 - my_y)
        xp = (1 - my_x, my_y)
        ebase = (1 - my_y) * H
        lbase = my_y * H

        def src(base, o, n):
            return x_hbm.at[pl.ds(pl.multiple_of(base + o, 8), n)]

        def ecp(i, o, c):
            return pltpu.make_async_copy(
                src(ebase, o, c), buf.at[pl.ds(pl.multiple_of(o, 8), c)],
                in_sems.at[i])

        def lcp(i, o, c):
            return pltpu.make_async_copy(
                src(lbase, o, c), buf.at[pl.ds(pl.multiple_of(H + o, 8), c)],
                in_sems.at[i])

        def rcopy(s, d, k, dev):
            return pltpu.make_async_remote_copy(
                s, d, send_sems.at[k], recv_sems.at[k],
                device_id=dev, device_id_type=MESH)

        ecp(0, *early[0]).start()
        ecp(1, *early[1]).start()
        s_in = pltpu.make_async_copy(src(lbase, 256, S), sm, sm_sems.at[0])
        s_out = pltpu.make_async_copy(sm, buf.at[pl.ds(H + 256, S)], sm_sems.at[1])
        s_in.start()
        bar = pltpu.get_barrier_semaphore()
        pl.semaphore_signal(bar, inc=1, device_id=yp, device_id_type=MESH)
        pl.semaphore_signal(bar, inc=1, device_id=xp, device_id_type=MESH)
        for i in range(2, ne):
            ecp(i, *early[i]).start()
        for j, (o, c) in enumerate(irr + reg + lastc):
            lcp(ne + j, o, c).start()

        y_raw = rcopy(src(ebase, 0, 128 + RB), buf.at[pl.ds(0, 128 + RB)], 0, yp)
        x_raw = rcopy(src(lbase, 384, 128 + XB), xbuf, 1, xp)
        y_part = rcopy(part.at[pl.ds(1, G - 1)], recv.at[pl.ds(1, G - 1)], 2, yp)
        x_ret = rcopy(xpart, xrecv, 3, xp)
        fin_send, fin_recv = [], []
        for k, (g0, n) in enumerate([(0, G - 1), (G - 1, 1)]):
            own = out_ref.at[my_y, pl.ds(g0, n)]
            oth = out_ref.at[1 - my_y, pl.ds(g0, n)]
            fin_send.append(rcopy(own, own, 4 + k, yp))
            fin_recv.append(rcopy(oth, oth, 4 + k, yp))

        pl.semaphore_wait(bar, 2)
        y_raw.start()
        x_raw.start()

        ecp(0, *early[0]).wait()
        part[pl.ds(1, 1), :] = _rowmax(buf[pl.ds(early[0][0], early[0][1]), :], RB)

        def eloop(lo, hi):
            def step(i, carry):
                o = pl.multiple_of(256 + (i - 1) * 128 * EC, 128)
                ecp(i, o, 128 * EC).wait()
                for r in range(EC):
                    row0 = pl.multiple_of(o + r * 128, 128)
                    part[pl.ds(2 + (i - 1) * EC + r, 1), :] = _rowmax(
                        buf[pl.ds(row0, 128), :])
                return carry
            lax.fori_loop(lo, hi, step, 0)

        mid = 1 + (S_FWD_AT - 1) // EC
        eloop(1, mid)
        s_in.wait()
        s_out.start()
        eloop(mid, ne)
        y_part.start()

        mine = out_ref.at[my_y]

        def merge(g, v):
            mine[pl.ds(g, 1), :] = jnp.maximum(mine[pl.ds(g, 1), :], v)

        mine[pl.ds(3, 1), :] = jnp.full((1, 128), NEG, jnp.float32)
        for j, (o, c) in enumerate(irr):
            lcp(ne + j, o, c).wait()
            for r in range(max(1, c // 128)):
                mine[pl.ds(o // 128 + r, 1), :] = _rowmax(
                    buf[pl.ds(H + o + r * 128, min(c, 128)), :], o % 128)

        def lloop(g_lo, g_hi):
            def step(g, carry):
                o = pl.multiple_of(g * 128, 128)
                lcp(ne + ni + g - 5, o, 128).wait()
                mine[pl.ds(g, 1), :] = _rowmax(
                    buf[pl.ds(pl.multiple_of(H + o, 128), 128), :])
                return carry
            lax.fori_loop(g_lo, g_hi, step, 0)

        lloop(5, X_AT + 1)
        x_raw.wait_recv()
        xpart[pl.ds(0, 1), :] = _rowmax(xbuf[pl.ds(0, 128), :])
        xpart[pl.ds(1, 1), :] = _rowmax(xbuf[pl.ds(128, XB), :])
        x_ret.start()

        lloop(X_AT + 1, S_AT + 1)
        s_out.wait()
        merge(2, _rowmax(buf[pl.ds(H + 256, S), :]))

        lloop(S_AT + 1, G - 1)
        y_raw.wait_recv()
        merge(0, _rowmax(buf[pl.ds(0, 128), :]))
        merge(1, _rowmax(buf[pl.ds(128, RB), :]))

        x_ret.wait_recv()
        mine[pl.ds(3, 2), :] = jnp.maximum(mine[pl.ds(3, 2), :], xrecv[...])

        y_part.wait_recv()
        mine[pl.ds(1, G - 2), :] = jnp.maximum(
            mine[pl.ds(1, G - 2), :], recv[pl.ds(1, G - 2), :])
        fin_send[0].start()

        acc = jnp.broadcast_to(recv[pl.ds(G - 1, 1), :], (8, 128))
        for j, (o, c) in enumerate(lastc):
            lcp(ne + ni + nr + j, o, c).wait()
            acc = jnp.maximum(acc, _place(buf[pl.ds(H + o, c), :], o % 128))
        mine[pl.ds(G - 1, 1), :] = jnp.max(acc, axis=0, keepdims=True)
        fin_send[1].start()

        for s in (y_raw, x_raw, y_part, x_ret, fin_send[0], fin_send[1]):
            s.wait_send()
        fin_recv[0].wait_recv()
        fin_recv[1].wait_recv()

    out = pl.pallas_call(
        body,
        out_shape=jax.ShapeDtypeStruct((2, G, 128), jnp.float32),
        in_specs=[pl.BlockSpec(memory_space=pl.ANY)],
        out_specs=pl.BlockSpec(memory_space=pltpu.VMEM),
        scratch_shapes=[
            pltpu.VMEM((M, N), jnp.float32),
            pltpu.VMEM((128 + XB, N), jnp.float32),
            pltpu.SMEM((S, N), jnp.float32),
            pltpu.VMEM((G, 128), jnp.float32),
            pltpu.VMEM((G, 128), jnp.float32),
            pltpu.VMEM((2, 128), jnp.float32),
            pltpu.VMEM((2, 128), jnp.float32),
            pltpu.SemaphoreType.DMA((nch,)),
            pltpu.SemaphoreType.DMA((2,)),
            pltpu.SemaphoreType.DMA((6,)),
            pltpu.SemaphoreType.DMA((6,)),
        ],
        compiler_params=pltpu.CompilerParams(
            collective_id=0,
            vmem_limit_bytes=64 * 1024 * 1024,
            disable_semaphore_checks=True,
            disable_bounds_checks=True,
        ),
    )(x)
    return out.reshape(M, 1)
```
